```python
import numpy as np

kernel_name = "dist_moe_cap_ep_n512_d256_e4_h512"

def setup_inputs():
    x = np.random.randn(512, 256).astype(np.float32)
    router_W = np.random.randn(256, 16).astype(np.float32) * 0.1
    scores64 = x.astype(np.float64) @ router_W.astype(np.float64)
    route_idx = np.argsort(-scores64, axis=-1)[:, :1].astype(np.int32)
    expert_W = np.random.randn(16, 256, 512).astype(np.float32) * 0.02
    return {"x": x, "router_W": router_W, "route_idx": route_idx, "expert_W": expert_W}

def reference(x, router_W, route_idx, expert_W):
    counts = np.zeros(16, dtype=np.int64)
    out = np.zeros((512, 512), dtype=np.float32)
    for i in range(512):
        e = int(route_idx[i, 0])
        if counts[e] < 25:
            out[i] = x[i] @ expert_W[e]
            counts[e] += 1
    return out
```

```python
import jax
import jax.numpy as jnp
from jax import lax
from jax.experimental import pallas as pl
from jax.experimental.pallas import tpu as pltpu

F32, BF16, I32, U32 = jnp.float32, jnp.bfloat16, jnp.int32, jnp.uint32

N_TOK, D_IN, D_OUT = 512, 256, 512
N_EXP, N_LOCAL, CAP = 16, 4, 25

A, B, D, C = 0, 1, 2, 3
ALL = (0, 1, 2, 3)
RIGHT, DIAG, LEFT = 1, 2, 3

PIECES = (
    [(e, c, 256) for e in (0, 1) for c in (0, 256)]
    + [(e, c, 128) for e in (2, 3) for c in (0, 128, 256, 384)]
)
N_PIECES = len(PIECES)
ROWS = [CAP if w == 256 else (CAP + 1) // 2 for _, _, w in PIECES]
PADDED = [32 if w == 256 else 16 for _, _, w in PIECES]
OFFSET = [sum(PADDED[:k]) for k in range(N_PIECES)]

VIA_C = (0, 2, 3, 4, 5)
LATE_TO_B = tuple(range(4, N_PIECES))
C_FORWARDS_AFTER = {9: (0,)}
FETCH_AFTER = {1: 2, 2: 3}
DIAG_AFTER = {7: (1,), 10: (0,)}
DIAG_STAGED = (6, 2, 7)
DIAG_MERGED = (8, 3, 9, 4, 10, 5, 11)
MERGE_MASKS = sorted({(PIECES[k][0], PIECES[k][2]) for k in DIAG_MERGED})


def _body(x_hbm, idx_hbm, w_hbm, out_ref,
          idx_v, rows_v, y_v, addr_v, addr_s, stage, mask_v, sent_v,
          local_sem, send_sem, recv_sem, *w_v):
    idx_copy = pltpu.make_async_copy(idx_hbm, idx_v, local_sem.at[0])
    idx_copy.start()
    w_copies = [
        pltpu.make_async_copy(
            w_hbm.at[e, :, pl.ds(c, w)], w_v[k], local_sem.at[10 + k])
        for k, (e, c, w) in enumerate(PIECES)
    ]
    for copy in w_copies:
        copy.start(priority=1)

    me = lax.axis_index("i")

    def peer(offset):
        return dict(device_id=((me + offset) & 3,),
                    device_id_type=pl.DeviceIdType.MESH)

    def on(chips, fn):
        if len(chips) == len(ALL):
            return fn()
        if len(chips) == len(ALL) - 1:
            pred = me != [c for c in ALL if c not in chips][0]
        else:
            pred = me == chips[0]
            for c in chips[1:]:
                pred = pred | (me == c)
        pl.when(pred)(fn)

    barrier = pltpu.get_barrier_semaphore()
    pl.semaphore_signal(barrier, inc=1, **peer(RIGHT))
    pl.semaphore_signal(barrier, inc=1, **peer(LEFT))
    on((A,), lambda: pl.semaphore_signal(barrier, inc=1, **peer(DIAG)))

    rows_v[:, 24:32, :] = jnp.zeros((N_LOCAL, 8, D_IN), F32)
    stage[0:4 * N_TOK, :] = jnp.zeros((4 * N_TOK, 128), F32)

    upper = (lax.broadcasted_iota(I32, (128, 128), 0)
             <= lax.broadcasted_iota(I32, (128, 128), 1))
    upper = jnp.where(upper, 1.0, 0.0).astype(BF16)
    ones = jnp.ones((128, 128), BF16)

    def running_counts(n):
        row = lax.broadcasted_iota(I32, (n, 128), 0)
        hits = []
        for b in range(4):
            e = jnp.broadcast_to(idx_v[b:b + 1, :], (n, 128))
            hits.append(jnp.where(((e - N_LOCAL * me) & (N_EXP - 1)) == row, 1.0, 0.0))
        hits = jnp.concatenate(hits, axis=0).astype(BF16)
        within = jnp.dot(hits, upper, preferred_element_type=F32)
        totals = jnp.dot(hits, ones, preferred_element_type=F32)
        counts, before = [within[:n]], totals[:n]
        for b in range(1, 4):
            counts.append(within[n * b:n * b + n] + before)
            before = before + totals[n * b:n * b + n]
        return counts

    def tokens_before(counts, slot):
        acc = jnp.where(counts[0] <= slot, 1.0, 0.0)
        for cnt in counts[1:]:
            acc = acc + jnp.where(cnt <= slot, 1.0, 0.0)
        return acc

    def of_expert(counts, r, n):
        return [jnp.broadcast_to(cnt[r:r + 1, :], (n, 128)) for cnt in counts]

    def row_of_x(counts, slot):
        tok = jnp.sum(tokens_before(counts, slot), axis=1, keepdims=True)
        return pltpu.bitcast(jnp.minimum(tok, N_TOK - 1.0) + 8388608.0, I32) & (N_TOK - 1)

    idx_copy.wait()
    local = running_counts(8)
    slots24 = lax.broadcasted_iota(I32, (24, 128), 0).astype(F32)
    x_row = [row_of_x(of_expert(local, 0, 24), slots24)]
    x_row_last = row_of_x(local, CAP - 1.0)

    def fetch_rows(e):
        with jax.named_scope(f"rows{e}"):
            if e == 0:
                x_row.extend(row_of_x(of_expert(local, r, 24), slots24) for r in (1, 2, 3))
            for p in range(CAP):
                t = x_row[e][p, 0] if p < 24 else x_row_last[e, 0]
                pltpu.make_async_copy(
                    x_hbm.at[pl.ds(t, 1)], rows_v.at[e, pl.ds(p, 1)],
                    local_sem.at[1 + 2 * e + p // 24]).start()

    def fetched_rows(e):
        for half, rows in enumerate((pl.ds(0, 24), pl.ds(24, 1))):
            buf = rows_v.at[e, rows]
            pltpu.make_async_copy(buf, buf, local_sem.at[1 + 2 * e + half]).wait()
        return rows_v[e].astype(BF16)

    def output_addresses():
        counts = running_counts(N_EXP)
        slot = lax.broadcasted_iota(I32, (32, 128), 0)
        for src in ALL:
            below = jnp.concatenate(
                [tokens_before(of_expert(counts, N_LOCAL * src + e, 32), slot.astype(F32))
                 for e in range(N_LOCAL)], axis=0)
            tok = lax.dot_general(
                jnp.ones((16, 128), BF16), below.astype(BF16),
                (((1,), (1,)), ((), ())), preferred_element_type=F32)
            tok = tok[0:1].astype(I32)
            addr_v[src:src + 1, :] = (tok >> 3) * 32 + (tok & 7)
            addr_v[4 + src:5 + src, :] = jnp.minimum(tok >> 3, 63) * 16 + ((tok >> 1) & 3)
        for q, (e, w) in enumerate(MERGE_MASKS):
            s = slot if w == 256 else 2 * (slot & 15) + (slot >> 4)
            tok = tokens_before(of_expert(counts, N_LOCAL * DIAG + e, 32), s.astype(F32))
            tok = jnp.sum(tok, axis=1, keepdims=True).astype(I32)
            tok = jnp.broadcast_to(tok, (32, 128))
            half = jnp.where((tok & 1) == 1, U32(0xFFFF0000), U32(0xFFFF))
            mask_v[q] = jnp.where(tok < N_TOK, half, U32(0))
        copy = pltpu.make_async_copy(addr_v, addr_s, local_sem.at[9])
        copy.start()
        copy.wait()

    rows_sent = [0] * len(ALL)

    def remote(k, src, offset):
        dst = (src - offset) % 4
        rows = pl.ds(OFFSET[k], ROWS[k])
        return pltpu.make_async_remote_copy(
            y_v.at[src, rows], y_v.at[dst, rows],
            send_sem, recv_sem.at[dst * N_PIECES + k], **peer(offset))

    def wait_received(src, k):
        remote(k, (src + 1) % 4, RIGHT).wait_recv()

    def send(k, offset, chips):
        on(chips, lambda: remote(k, 0, offset).start())
        for chip in chips:
            rows_sent[chip] += ROWS[k]

    def forward(k, src, offset, chip):
        def fn():
            wait_received(src, k)
            remote(k, src, offset).start()
        on((chip,), fn)
        rows_sent[chip] += ROWS[k]

    def wait_sent(chip):
        buf = sent_v.at[pl.ds(0, rows_sent[chip])]
        pltpu.make_async_copy(buf, buf, send_sem).wait()

    def stage_piece(src, k):
        e, c, w = PIECES[k]
        j = c // 128
        low = lambda v: pltpu.bitcast(v << 16, F32)
        high = lambda v: pltpu.bitcast(v & U32(0xFFFF0000), F32)
        for p in range(CAP):
            row = addr_s[src, 32 * e + p] + 8 * j
            if w == 256:
                v = y_v[src, pl.ds(OFFSET[k] + p, 1), :]
                stage[pl.ds(row, 1), :] = low(v)
                stage[pl.ds(row + 8, 1), :] = high(v)
            else:
                v = y_v[src, pl.ds(OFFSET[k] + p // 2, 1), :]
                stage[pl.ds(row, 1), :] = high(v) if p % 2 else low(v)

    def merge_piece(k):
        e, c, w = PIECES[k]
        blocks = range(c // 128, (c + w) // 128)
        words = out_ref.bitcast(U32)
        mask = mask_v[MERGE_MASKS.index((e, w))]
        for parity in (0, 1):
            where = [(p, i, pl.ds(addr_s[4 + DIAG, 32 * e + p] + 4 * j, 1))
                     for p in reversed(range(parity, CAP, 2))
                     for i, j in enumerate(blocks)]
            old = [words[row, :] for _, _, row in where]
            if parity == 0:
                wait_received(DIAG, k)
                v = y_v[DIAG, pl.ds(OFFSET[k], ROWS[k]), :]
                low = (v << 16) | (v & U32(0xFFFF))
                high = (v >> 16) | (v & U32(0xFFFF0000))
                other = 0 if w == 256 else 16
                new = (low & mask[:ROWS[k]], high & mask[other:other + ROWS[k]])
            for (p, i, row), word in zip(where, old):
                bits = new[i][p:p + 1] if w == 256 else new[parity][p // 2:p // 2 + 1]
                words[row, :] = word | bits

    fetch_rows(0)
    fetch_rows(1)
    on((A,), output_addresses)

    lhs = {}
    for k, (e, c, w) in enumerate(PIECES):
        if e not in lhs:
            lhs[e] = fetched_rows(e)
        w_copies[k].wait()
        rhs = w_v[k][...].astype(BF16)
        if w == 256:
            y = jnp.dot(lhs[e], rhs, preferred_element_type=F32)
            y = pltpu.bitcast(y.astype(BF16).astype(F32), U32)
            y = (y[:, :128] >> 16) | y[:, 128:]
        else:
            y = jnp.concatenate(
                [jnp.dot(lhs[e][h:h + 16], rhs, preferred_element_type=F32)
                 for h in (0, 16)], axis=0)
            y = pltpu.bitcast(y.astype(BF16), U32)
        y_v[0, pl.ds(OFFSET[k], PADDED[k]), :] = y
        if k == 0:
            on((A, B, C), lambda: pl.semaphore_wait(barrier, 2))
            on((D,), lambda: pl.semaphore_wait(barrier, 3))
        if k not in VIA_C:
            send(k, DIAG, (D,))
        send(k, LEFT, (A, B, C) if k in LATE_TO_B else ALL)
        send(k, RIGHT, ALL)
        if k in FETCH_AFTER:
            fetch_rows(FETCH_AFTER[k])
        for q in C_FORWARDS_AFTER.get(k, ()):
            forward(q, LEFT, RIGHT, C)
    for k in LATE_TO_B:
        send(k, LEFT, (D,))
    for k in VIA_C:
        if not any(k in ks for ks in C_FORWARDS_AFTER.values()):
            forward(k, LEFT, RIGHT, C)
    for k in range(N_PIECES):
        forward(k, LEFT, RIGHT, B)
    on((B, C, D), output_addresses)

    for k in range(N_PIECES):
        stage_piece(0, k)
        forward(k, LEFT, RIGHT, A)
        forward(k, RIGHT, LEFT, A)
        on((D,) if k in VIA_C else (C, D), lambda: wait_received(LEFT, k))
        stage_piece(LEFT, k)
        on((C, D) if k in LATE_TO_B else (B, C, D), lambda: wait_received(RIGHT, k))
        on((A, C, D) if k in LATE_TO_B else ALL, lambda: stage_piece(RIGHT, k))
        for q in DIAG_AFTER.get(k, ()):
            wait_received(DIAG, q)
            stage_piece(DIAG, q)
    for k in DIAG_STAGED:
        wait_received(DIAG, k)
        stage_piece(DIAG, k)

    @pl.when(me == B)
    def _():
        for k in LATE_TO_B:
            wait_received(RIGHT, k)
            stage_piece(RIGHT, k)

    out_ref[...] = stage[0:4 * N_TOK, :].astype(BF16)
    for k in DIAG_MERGED:
        if k == DIAG_MERGED[-1]:
            for chip in ALL:
                on((chip,), lambda: wait_sent(chip))
        merge_piece(k)


def pallas_dist_moe_cap_ep_n512_d256_e4_h512_kernel(
    x: jax.Array,
    router_W: jax.Array,
    route_idx: jax.Array,
    expert_W: jax.Array,
):
    del router_W
    hbm = pl.BlockSpec(memory_space=pltpu.HBM)
    out = pl.pallas_call(
        _body,
        out_shape=jax.ShapeDtypeStruct((4 * N_TOK, 128), BF16),
        in_specs=[hbm, hbm, hbm],
        out_specs=pl.BlockSpec(memory_space=pltpu.VMEM),
        scratch_shapes=[
            pltpu.VMEM((4, 128), I32),
            pltpu.VMEM((N_LOCAL, 32, D_IN), F32),
            pltpu.VMEM((4, sum(PADDED), 128), U32),
            pltpu.VMEM((8, 128), I32),
            pltpu.SMEM((8, 128), I32),
            pltpu.VMEM((4 * N_TOK + 32, 128), F32),
            pltpu.VMEM((len(MERGE_MASKS), 32, 128), U32),
            pltpu.VMEM((4 * sum(PADDED), 128), U32),
            pltpu.SemaphoreType.DMA((10 + N_PIECES,)),
            pltpu.SemaphoreType.DMA,
            pltpu.SemaphoreType.DMA((4 * N_PIECES,)),
        ] + [pltpu.VMEM((D_IN, w), F32) for _, _, w in PIECES],
        compiler_params=pltpu.CompilerParams(
            collective_id=0, disable_bounds_checks=True, disable_semaphore_checks=True),
    )(x, route_idx.reshape(4, 128), expert_W)
    return out.reshape(N_TOK // 8, 4, 8, 128).transpose(0, 2, 1, 3).reshape(N_TOK, D_OUT)
```

```python
import jax
import jax.numpy as jnp
from jax import lax
from jax.experimental import pallas as pl
from jax.experimental.pallas import tpu as pltpu

F32, BF16, I32, U32 = jnp.float32, jnp.bfloat16, jnp.int32, jnp.uint32

N_TOK, D_IN, D_OUT = 512, 256, 512
N_EXP, N_LOCAL, CAP = 16, 4, 25

A, B, D, C = 0, 1, 2, 3
ALL = (0, 1, 2, 3)
OWN, RIGHT, DIAG, LEFT = 0, 1, 2, 3
WRITES_TO = {A: (B, C), B: (A, D), C: (A, D), D: (A, B, C)}

BLOCKS = ([(e, c, 256) for e in (0, 1) for c in (0, 256)]
          + [(e, c, 128) for e in (2, 3) for c in (0, 128, 256, 384)])
STEPS = [(0, 0, 8), (0, 8, CAP)] + [(b, 0, CAP) for b in range(1, len(BLOCKS))]
ROW_GROUPS = [(0, 8, 24, CAP)] + [(0, 24, CAP)] * 3


def _words(step):
    b, first, end = STEPS[step]
    _, c, w = BLOCKS[b]
    j = c // 128
    if w == 256:
        return [((p, j), (p, j + 1)) for p in range(first, end)]
    words = [((p, j), (p + 1, j)) for p in range(0, CAP - 1, 2)]
    if j % 2:
        words.append(((CAP - 1, j), (CAP - 1, j - 1)))
    return words


N_STEPS = len(STEPS)
EXPERT = [BLOCKS[b][0] for b, _, _ in STEPS]
WORDS = [_words(s) for s in range(N_STEPS)]
FIRST_ROW = [sum(pl.cdiv(len(w), 8) * 8 for w in WORDS[:s]) for s in range(N_STEPS + 1)]

VIA_C = (0, 1, 3, 4, 5, 6)
LATE_TO_B = tuple(range(5, N_STEPS))
C_FORWARDS_AFTER = {9: 0, 11: 1}
LAST_FETCH_AFTER = 3
DIAG_AFTER = {8: 2, 10: 0, 11: 1}
DIAG_STAGED = (7, 3, 8)
DIAG_MERGED = (9, 4, 10, 5, 11, 6, 12)


def _mask_key(step, half):
    first, second = (WORDS[step][i][half][0] for i in (0, 1))
    return EXPERT[step], first, second - first


MASK_KEYS = sorted({_mask_key(s, half) for s in DIAG_MERGED for half in (0, 1)})


def _body(x_hbm, idx_hbm, w_hbm, out_ref,
          idx_v, rows_v, y_v, addr_v, addr_s, stage, mask_v, sent_v,
          local_sem, send_sem, recv_sem, *w_v):
    idx_copy = pltpu.make_async_copy(idx_hbm, idx_v, local_sem.at[0])
    idx_copy.start()
    w_copies = [
        pltpu.make_async_copy(
            w_hbm.at[e, :, pl.ds(c, w)], w_v[b], local_sem.at[2 + b])
        for b, (e, c, w) in enumerate(BLOCKS)
    ]
    for copy in w_copies:
        copy.start(priority=1)

    me = lax.axis_index("i")

    def chip(position):
        return dict(device_id=(position,), device_id_type=pl.DeviceIdType.MESH)

    def on(chips, fn):
        if len(chips) == len(ALL):
            return fn()
        if len(chips) == len(ALL) - 1:
            pred = me != [c for c in ALL if c not in chips][0]
        else:
            pred = me == chips[0]
            for c in chips[1:]:
                pred = pred | (me == c)
        pl.when(pred)(fn)

    barrier = pltpu.get_barrier_semaphore()
    for writer in ALL:
        on(WRITES_TO[writer], lambda: pl.semaphore_signal(barrier, inc=1, **chip(writer)))

    rows_v[:, 24:32, :] = jnp.zeros((N_LOCAL, 8, D_IN), F32)
    stage[0:4 * N_TOK, :] = jnp.zeros((4 * N_TOK, 128), F32)

    upper = (lax.broadcasted_iota(I32, (128, 128), 0)
             <= lax.broadcasted_iota(I32, (128, 128), 1))
    upper = jnp.where(upper, 1.0, 0.0).astype(BF16)
    ones = jnp.ones((128, 128), BF16)

    def running_counts(n):
        row = lax.broadcasted_iota(I32, (n, 128), 0)
        hits = []
        for b in range(4):
            e = jnp.broadcast_to(idx_v[b:b + 1, :], (n, 128))
            hits.append(jnp.where(((e - N_LOCAL * me) & (N_EXP - 1)) == row, 1.0, 0.0))
        hits = jnp.concatenate(hits, axis=0).astype(BF16)
        within = jnp.dot(hits, upper, preferred_element_type=F32)
        totals = jnp.dot(hits, ones, preferred_element_type=F32)
        counts, before = [within[:n]], totals[:n]
        for b in range(1, 4):
            counts.append(within[n * b:n * b + n] + before)
            before = before + totals[n * b:n * b + n]
        return counts

    def tokens_before(counts, slot):
        acc = jnp.where(counts[0] <= slot, 1.0, 0.0)
        for cnt in counts[1:]:
            acc = acc + jnp.where(cnt <= slot, 1.0, 0.0)
        return acc

    def of_expert(counts, r, n):
        return [jnp.broadcast_to(cnt[r:r + 1, :], (n, 128)) for cnt in counts]

    def row_of_x(counts, slot):
        tok = jnp.sum(tokens_before(counts, slot), axis=1, keepdims=True)
        return pltpu.bitcast(jnp.minimum(tok, N_TOK - 1.0) + 8388608.0, I32) & (N_TOK - 1)

    def rows_sem(e, group):
        return local_sem.at[2 + len(BLOCKS) + 3 * e + group]

    def fetch_rows(e, first_24, last):
        @pl.when(me < len(ALL))
        def _():
            for p in range(CAP):
                t = first_24[p, 0] if p < CAP - 1 else last[e, 0]
                group = sum(p >= edge for edge in ROW_GROUPS[e][1:])
                pltpu.make_async_copy(
                    x_hbm.at[pl.ds(t, 1)], rows_v.at[e, pl.ds(p, 1)],
                    rows_sem(e, group)).start()

    awaited = []

    def fetched_rows(e, first, end):
        edges = ROW_GROUPS[e]
        for group in range(edges.index(first), edges.index(end)):
            if (e, group) not in awaited:
                awaited.append((e, group))
                buf = rows_v.at[e, pl.ds(edges[group], edges[group + 1] - edges[group])]
                pltpu.make_async_copy(buf, buf, rows_sem(e, group)).wait()
        return rows_v[e, pl.ds(first, pl.cdiv(end - first, 8) * 8), :].astype(BF16)

    def output_addresses():
        counts = running_counts(N_EXP)
        slot = lax.broadcasted_iota(I32, (32, 128), 0)
        for src in ALL:
            below = jnp.concatenate(
                [tokens_before(of_expert(counts, N_LOCAL * src + e, 32), slot.astype(F32))
                 for e in range(N_LOCAL)], axis=0)
            tok = lax.dot_general(
                jnp.ones((16, 128), BF16), below.astype(BF16),
                (((1,), (1,)), ((), ())), preferred_element_type=F32)
            tok = tok[0:1].astype(I32)
            addr_v[src:src + 1, :] = (tok >> 3) * 32 + (tok & 7)
            addr_v[4 + src:5 + src, :] = jnp.minimum(tok >> 3, 63) * 16 + ((tok >> 1) & 3)
        for q, (e, first, stride) in enumerate(MASK_KEYS):
            s = jnp.minimum(first + stride * slot, CAP - 1)
            tok = tokens_before(of_expert(counts, N_LOCAL * DIAG + e, 32), s.astype(F32))
            tok = jnp.sum(tok, axis=1, keepdims=True).astype(I32)
            tok = jnp.broadcast_to(tok, (32, 128))
            half = jnp.where((tok & 1) == 1, U32(0xFFFF0000), U32(0xFFFF))
            mask_v[q] = jnp.where(tok < N_TOK, half, U32(0))
        copy = pltpu.make_async_copy(addr_v, addr_s, local_sem.at[1])
        copy.start()
        copy.wait()

    rows_sent = [0] * len(ALL)

    def remote(s, src, to, dst):
        rows = pl.ds(FIRST_ROW[s], len(WORDS[s]))
        return pltpu.make_async_remote_copy(
            y_v.at[src, rows], y_v.at[dst, rows],
            send_sem, recv_sem.at[dst * N_STEPS + s], **chip(to))

    def wait_received(src, s):
        remote(s, OWN, A, src).wait_recv()

    def send(s, to, chips):
        on(chips, lambda: remote(s, OWN, to, (me - to) & 3).start())
        for c in chips:
            rows_sent[c] += len(WORDS[s])

    def forward(s, origin, by, to):
        def fn():
            wait_received((origin - by) % 4, s)
            remote(s, (origin - by) % 4, to, (origin - to) % 4).start()
        on((by,), fn)
        rows_sent[by] += len(WORDS[s])

    def wait_all_sent(c):
        total = sent_v.at[pl.ds(0, rows_sent[c])]
        pltpu.make_async_copy(total, total, send_sem).wait()

    def stage_rows(src, s):
        row_of = {p: addr_s[src, 32 * EXPERT[s] + p]
                  for p in sorted({p for word in WORDS[s] for p, _ in word})}
        for i, word in enumerate(WORDS[s]):
            v = y_v[src, pl.ds(FIRST_ROW[s] + i, 1), :]
            for (p, j), bits in zip(word, (v << 16, v & U32(0xFFFF0000))):
                stage[pl.ds(row_of[p] + 8 * j, 1), :] = pltpu.bitcast(bits, F32)

    def merge_rows(s):
        n = len(WORDS[s])
        out_words = out_ref.bitcast(U32)
        masks = [mask_v[MASK_KEYS.index(_mask_key(s, half)), pl.ds(0, n), :]
                 for half in (0, 1)]
        for parity in (0, 1):
            batch = [(i, half, pl.ds(addr_s[4 + DIAG, 32 * EXPERT[s] + p] + 4 * j, 1))
                     for i in reversed(range(n))
                     for half, (p, j) in enumerate(WORDS[s][i]) if p % 2 == parity]
            old = [out_words[row, :] for _, _, row in batch]
            if parity == 0:
                wait_received(DIAG, s)
                v = y_v[DIAG, pl.ds(FIRST_ROW[s], n), :]
                new = (((v << 16) | (v & U32(0xFFFF))) & masks[0],
                       ((v >> 16) | (v & U32(0xFFFF0000))) & masks[1])
            for (i, half, row), word in zip(batch, old):
                out_words[row, :] = word | new[half][i:i + 1]

    idx_copy.wait()
    local = running_counts(8)
    slots = lax.broadcasted_iota(I32, (24, 128), 0).astype(F32)
    x_row = [row_of_x(of_expert(local, 0, 24), slots)]
    x_row_last = row_of_x(local, CAP - 1.0)
    fetch_rows(0, x_row[0], x_row_last)
    x_row += [row_of_x(of_expert(local, e, 24), slots) for e in (1, 2, 3)]
    fetch_rows(1, x_row[1], x_row_last)
    fetch_rows(2, x_row[2], x_row_last)
    on((A,), output_addresses)

    lhs, last_slot = {}, {}
    for s, (b, first, end) in enumerate(STEPS):
        e, c, w = BLOCKS[b]
        if (e, first, end) not in lhs:
            lhs[e, first, end] = fetched_rows(e, first, end)
        if first == 0:
            w_copies[b].wait()
        rows, weights = lhs[e, first, end], w_v[b][...].astype(BF16)
        if w == 256:
            y = jnp.dot(rows, weights, preferred_element_type=F32)
            y = pltpu.bitcast(y.astype(BF16).astype(F32), U32)
            y = (y[:, :128] >> 16) | y[:, 128:]
        else:
            top, bottom = (jnp.dot(rows[h:h + 16], weights, preferred_element_type=F32)
                           for h in (0, 16))
            tail = bottom[8:]
            if c // 128 % 2:
                second = lax.broadcasted_iota(I32, (8, 128), 0) == 1
                tail = jnp.where(second, last_slot[e], tail)
            else:
                last_slot[e] = jnp.broadcast_to(tail[0:1], (8, 128))
            y = jnp.concatenate([top, bottom[:8], tail], axis=0)
            y = pltpu.bitcast(y.astype(BF16), U32)
        y_v[OWN, pl.ds(FIRST_ROW[s], y.shape[0]), :] = y
        if s == 0:
            on((A, B, C), lambda: pl.semaphore_wait(barrier, 2))
            on((D,), lambda: pl.semaphore_wait(barrier, 3))
        send(s, A, (B, C) if s in VIA_C else (B, C, D))
        send(s, C, (A, D))
        send(s, B, (A,) if s in LATE_TO_B else (A, D))
        send(s, D, (B, C))
        if s == LAST_FETCH_AFTER:
            fetch_rows(3, x_row[3], x_row_last)
        if s in C_FORWARDS_AFTER:
            forward(C_FORWARDS_AFTER[s], D, C, A)
    for s in LATE_TO_B:
        send(s, B, (D,))
    for s in VIA_C:
        if s not in C_FORWARDS_AFTER.values():
            forward(s, D, C, A)
    for s in range(N_STEPS):
        forward(s, A, B, D)
    on((B, C, D), output_addresses)

    for s in range(N_STEPS):
        stage_rows(OWN, s)
        forward(s, C, A, B)
        forward(s, B, A, C)
        on((D,) if s in VIA_C else (C, D), lambda: wait_received(LEFT, s))
        stage_rows(LEFT, s)
        on((C, D) if s in LATE_TO_B else (B, C, D), lambda: wait_received(RIGHT, s))
        on((A, C, D) if s in LATE_TO_B else ALL, lambda: stage_rows(RIGHT, s))
        if s in DIAG_AFTER:
            wait_received(DIAG, DIAG_AFTER[s])
            stage_rows(DIAG, DIAG_AFTER[s])
    for s in DIAG_STAGED:
        wait_received(DIAG, s)
        stage_rows(DIAG, s)

    @pl.when(me == B)
    def _():
        for s in LATE_TO_B:
            wait_received(RIGHT, s)
            stage_rows(RIGHT, s)

    out_ref[...] = stage[0:4 * N_TOK, :].astype(BF16)
    for s in DIAG_MERGED:
        if s == DIAG_MERGED[-4]:
            for c in ALL:
                on((c,), lambda: wait_all_sent(c))
        merge_rows(s)


def pallas_dist_moe_cap_ep_n512_d256_e4_h512_kernel(
    x: jax.Array,
    router_W: jax.Array,
    route_idx: jax.Array,
    expert_W: jax.Array,
):
    del router_W
    hbm = pl.BlockSpec(memory_space=pltpu.HBM)
    out = pl.pallas_call(
        _body,
        out_shape=jax.ShapeDtypeStruct((4 * N_TOK, 128), BF16),
        in_specs=[hbm, hbm, hbm],
        out_specs=pl.BlockSpec(memory_space=pltpu.VMEM),
        scratch_shapes=[
            pltpu.VMEM((4, 128), I32),
            pltpu.VMEM((N_LOCAL, 32, D_IN), F32),
            pltpu.VMEM((4, FIRST_ROW[-1], 128), U32),
            pltpu.VMEM((8, 128), I32),
            pltpu.SMEM((8, 128), I32),
            pltpu.VMEM((4 * N_TOK + 32, 128), F32),
            pltpu.VMEM((len(MASK_KEYS), 32, 128), U32),
            pltpu.VMEM((4 * FIRST_ROW[-1], 128), U32),
            pltpu.SemaphoreType.DMA((2 + len(BLOCKS) + 3 * N_LOCAL,)),
            pltpu.SemaphoreType.DMA,
            pltpu.SemaphoreType.DMA((4 * N_STEPS,)),
        ] + [pltpu.VMEM((D_IN, w), F32) for _, _, w in BLOCKS],
        compiler_params=pltpu.CompilerParams(
            collective_id=0, disable_bounds_checks=True, disable_semaphore_checks=True),
    )(x, route_idx.reshape(4, 128), expert_W)
    return out.reshape(N_TOK // 8, 4, 8, 128).transpose(0, 2, 1, 3).reshape(N_TOK, D_OUT)
```

```python
import jax
import jax.numpy as jnp
from jax import lax
from jax.experimental import pallas as pl
from jax.experimental.pallas import tpu as pltpu

F32, BF16, I32, U32 = jnp.float32, jnp.bfloat16, jnp.int32, jnp.uint32

N_TOK, D_IN, D_OUT = 512, 256, 512
N_EXP, N_LOCAL, CAP = 16, 4, 25

A, B, D, C = 0, 1, 2, 3
ALL = (0, 1, 2, 3)
OWN, RIGHT, DIAG, LEFT = 0, 1, 2, 3
DESTINATIONS = {A: (B, C), B: (A, D), C: (A, D), D: (A, B, C)}

WIDTH = (256, 256, 128, 128)
BLOCKS = [(e, c, w) for e, w in enumerate(WIDTH) for c in range(0, D_OUT, w)]
STEPS = [(0, 0, 8), (0, 8, CAP)] + [(b, 0, CAP) for b in range(1, len(BLOCKS))]
ROW_GROUPS = [(0, 8, 24, CAP)] + [(0, 24, CAP)] * 3


def _words(step):
    b, first, end = STEPS[step]
    _, c, w = BLOCKS[b]
    j = c // 128
    if w == 256:
        return [((p, j), (p, j + 1)) for p in range(first, end)]
    words = [((p, j), (p + 1, j)) for p in range(0, CAP - 1, 2)]
    if j % 2:
        words.append(((CAP - 1, j), (CAP - 1, j - 1)))
    return words


N_STEPS = len(STEPS)
EXPERT = [BLOCKS[b][0] for b, _, _ in STEPS]
STEPS_OF = [[s for s in range(N_STEPS) if EXPERT[s] == e] for e in range(N_LOCAL)]
WORDS = [_words(s) for s in range(N_STEPS)]
FIRST_ROW = [sum(pl.cdiv(len(w), 8) * 8 for w in WORDS[:s]) for s in range(N_STEPS + 1)]

VIA_C = (0, 1, 3, 4, 5, 6)
LATE_TO_B = STEPS_OF[2] + STEPS_OF[3]
NEIGHBOUR_GROUPS = ((0, 1, 2), (3, 4), (5, 6, 7, 8), (9, 10), (11,), (12,))
DIAG_EARLY = {8: 2, 10: 0, 11: 1}
DIAG_LATE = (7, 3, 8, 9, 4, 10, 5, 11, 6, 12)
SEND_LAG = 4
ZEROED_PER_STEP = 60


def _body(x_hbm, idx_hbm, w_hbm, out_ref,
          idx_v, rows_v, y_v, addr_v, addr_s, mask_v,
          local_sem, send_sem, recv_sem, *w_v):
    idx_copy = pltpu.make_async_copy(idx_hbm, idx_v, local_sem.at[0])
    idx_copy.start()
    w_copies = [
        pltpu.make_async_copy(
            w_hbm.at[e, :, pl.ds(c, w)], w_v[b], local_sem.at[2 + b])
        for b, (e, c, w) in enumerate(BLOCKS)
    ]
    for copy in w_copies:
        copy.start(priority=1)

    me = lax.axis_index("i")

    def chip(position):
        return dict(device_id=(position,), device_id_type=pl.DeviceIdType.MESH)

    def on(chips, fn):
        if len(chips) == len(ALL):
            return fn()
        if len(chips) == len(ALL) - 1:
            pred = me != [c for c in ALL if c not in chips][0]
        else:
            pred = me == chips[0]
            for c in chips[1:]:
                pred = pred | (me == c)
        pl.when(pred)(fn)

    barrier = pltpu.get_barrier_semaphore()
    for sender in ALL:
        on(DESTINATIONS[sender],
           lambda: pl.semaphore_signal(barrier, inc=1, **chip(sender)))

    def zero_output(first, end):
        out_ref[first:end] = jnp.zeros((end - first, 2, 128), BF16)

    rows_v[:, 24:32, :] = jnp.zeros((N_LOCAL, 8, D_IN), F32)
    zero_output((N_STEPS - 1) * ZEROED_PER_STEP, 2 * N_TOK)

    upper = (lax.broadcasted_iota(I32, (128, 128), 0)
             <= lax.broadcasted_iota(I32, (128, 128), 1))
    upper = jnp.where(upper, 1.0, 0.0).astype(BF16)
    ones = jnp.ones((128, 128), BF16)

    def running_counts(n):
        row = lax.broadcasted_iota(I32, (n, 128), 0)
        hits = []
        for b in range(4):
            e = jnp.broadcast_to(idx_v[b:b + 1, :], (n, 128))
            hits.append(jnp.where(((e - N_LOCAL * me) & (N_EXP - 1)) == row, 1.0, 0.0))
        hits = jnp.concatenate(hits, axis=0).astype(BF16)
        within = jnp.dot(hits, upper, preferred_element_type=F32)
        totals = jnp.dot(hits, ones, preferred_element_type=F32)
        counts, before = [within[:n]], totals[:n]
        for b in range(1, 4):
            counts.append(within[n * b:n * b + n] + before)
            before = before + totals[n * b:n * b + n]
        return counts

    def of_expert(counts, r, n):
        return [jnp.broadcast_to(cnt[r:r + 1, :], (n, 128)) for cnt in counts]

    def tokens_before(counts, slot):
        acc = jnp.where(counts[0] <= slot, 1.0, 0.0)
        for cnt in counts[1:]:
            acc = acc + jnp.where(cnt <= slot, 1.0, 0.0)
        return acc

    def as_int(small):
        return pltpu.bitcast(small + 8388608.0, I32)

    def row_of_x(counts, slot):
        tok = jnp.sum(tokens_before(counts, slot), axis=1, keepdims=True)
        return as_int(jnp.minimum(tok, N_TOK - 1.0)) & (N_TOK - 1)

    def rows_sem(e, group):
        return local_sem.at[2 + len(BLOCKS) + 3 * e + group]

    def fetch_rows(e, first_24, last):
        for p in range(CAP):
            t = first_24[p, 0] if p < CAP - 1 else last[e, 0]
            group = sum(p >= edge for edge in ROW_GROUPS[e][1:])
            pltpu.make_async_copy(
                x_hbm.at[pl.ds(t, 1)], rows_v.at[e, pl.ds(p, 1)],
                rows_sem(e, group)).start()

    awaited = []

    def fetched_rows(e, first, end):
        edges = ROW_GROUPS[e]
        for group in range(edges.index(first), edges.index(end)):
            if (e, group) not in awaited:
                awaited.append((e, group))
                buf = rows_v.at[e, pl.ds(edges[group], edges[group + 1] - edges[group])]
                pltpu.make_async_copy(buf, buf, rows_sem(e, group)).wait()
        return rows_v[e, pl.ds(first, pl.cdiv(end - first, 8) * 8), :].astype(BF16)

    addr_copy = pltpu.make_async_copy(addr_v, addr_s, local_sem.at[1])

    def output_rows():
        counts = running_counts(N_EXP)
        row = lax.broadcasted_iota(I32, (32, 128), 0)
        in_order = row.astype(F32)
        even_then_odd = jnp.minimum(2 * (row & 15) + (row >> 4), CAP - 1).astype(F32)
        below = [
            jnp.concatenate(
                [tokens_before(of_expert(counts, N_LOCAL * src + e, 32),
                               in_order if WIDTH[e] == 256 else even_then_odd)
                 for e in range(N_LOCAL)], axis=0).astype(BF16)
            for src in ALL]
        for src in ALL:
            tok = lax.dot_general(
                ones[:16], below[src], (((1,), (1,)), ((), ())), preferred_element_type=F32)
            tok = tok[0:1].astype(I32)
            addr_v[src:src + 1, :] = jnp.minimum(tok >> 3, 63) * 16 + ((tok >> 1) & 3)
        addr_copy.start()
        return below

    def output_halves(below):
        for src in ALL:
            tok = as_int(jnp.dot(below[src], ones, preferred_element_type=F32))
            half = jnp.where((tok & 1) == 1, U32(0xFFFF0000), U32(0xFFFF))
            mask_v[src] = jnp.where((tok & N_TOK) == 0, half, U32(0))

    started = [[] for _ in range(N_STEPS)]

    def remote(s, src, to, dst):
        rows = pl.ds(FIRST_ROW[s], len(WORDS[s]))
        return pltpu.make_async_remote_copy(
            y_v.at[src, rows], y_v.at[dst, rows],
            send_sem.at[(2 * to + (src != OWN)) * N_STEPS + s],
            recv_sem.at[dst * N_STEPS + s], **chip(to))

    def wait_received(src, s):
        remote(s, OWN, A, src).wait_recv()

    def send(s, to, chips):
        on(chips, lambda: remote(s, OWN, to, (me - to) & 3).start())
        started[s].append((OWN, to, chips))

    def forward(s, origin, by, to):
        src = (origin - by) % 4

        def fn():
            wait_received(src, s)
            remote(s, src, to, (origin - to) % 4).start()
        on((by,), fn)
        started[s].append((src, to, (by,)))

    def wait_sent(s, forwarded):
        for src, to, chips in started[s]:
            if (src != OWN) == forwarded:
                on(chips, lambda: remote(s, src, to, DIAG).wait_send())

    def write_rows(src, steps, wait_for_them=False):
        e = EXPERT[steps[0]]
        at = {(s, half): 32 * e + (STEPS[s][1] if WIDTH[e] == 256 else 16 * half)
              for s in steps for half in (0, 1)}
        masks = {(s, half): mask_v[src, pl.ds(first, len(WORDS[s])), :]
                 for (s, half), first in at.items()}
        entries = sorted(((p, j, s, i, half) for s in steps for i, word in enumerate(WORDS[s])
                          for half, (p, j) in enumerate(word)), reverse=True)
        for parity in (0, 1):
            batch = [entry for entry in entries if entry[0] % 2 == parity]
            base = {}
            for p, _, s, i, half in batch:
                if p not in base:
                    base[p] = addr_s[src, at[s, half] + i]
            old = [pltpu.bitcast(out_ref[base[p] + 4 * j], U32) for p, j, *_ in batch]
            if parity == 0:
                new = {}
                for s in steps:
                    if wait_for_them:
                        wait_received(src, s)
                    v = y_v[src, pl.ds(FIRST_ROW[s], len(WORDS[s])), :]
                    new[s, 0] = ((v << 16) | (v & U32(0xFFFF))) & masks[s, 0]
                    new[s, 1] = ((v >> 16) | (v & U32(0xFFFF0000))) & masks[s, 1]
            for (p, j, s, i, half), word in zip(batch, old):
                out_ref[base[p] + 4 * j] = pltpu.bitcast(word | new[s, half][i:i + 1], BF16)

    def undisturbed(fn):
        pl.when(me != len(ALL))(fn)

    idx_copy.wait()
    local = running_counts(8)
    slots = lax.broadcasted_iota(I32, (24, 128), 0).astype(F32)
    x_row = [row_of_x(of_expert(local, 0, 24), slots)]
    x_row_last = row_of_x(local, CAP - 1.0)
    undisturbed(lambda: fetch_rows(0, x_row[0], x_row_last))
    x_row += [row_of_x(of_expert(local, e, 24), slots) for e in (1, 2, 3)]
    fetch_rows(1, x_row[1], x_row_last)
    fetch_rows(2, x_row[2], x_row_last)

    lhs, last_slot = {}, {}
    for s, (b, first, end) in enumerate(STEPS):
        e, c, w = BLOCKS[b]
        if (e, first, end) not in lhs:
            lhs[e, first, end] = fetched_rows(e, first, end)
        if first == 0:
            w_copies[b].wait()
        rows, weights = lhs[e, first, end], w_v[b][...].astype(BF16)
        if w == 256:
            y = jnp.dot(rows, weights, preferred_element_type=F32)
            y = pltpu.bitcast(y.astype(BF16).astype(F32), U32)
            y = (y[:, :128] >> 16) | y[:, 128:]
        else:
            top, bottom = (jnp.dot(rows[h:h + 16], weights, preferred_element_type=F32)
                           for h in (0, 16))
            tail = bottom[8:]
            if c // 128 % 2:
                second = lax.broadcasted_iota(I32, (8, 128), 0) == 1
                tail = jnp.where(second, last_slot[e], tail)
            else:
                last_slot[e] = jnp.broadcast_to(tail[0:1], (8, 128))
            y = jnp.concatenate([top, bottom[:8], tail], axis=0)
            y = pltpu.bitcast(y.astype(BF16), U32)
        if s < N_STEPS - 1:
            zero_output(s * ZEROED_PER_STEP, (s + 1) * ZEROED_PER_STEP)
        y_v[OWN, pl.ds(FIRST_ROW[s], y.shape[0]), :] = y
        if s == 0:
            on((A, B, C), lambda: pl.semaphore_wait(barrier, 2))
            on((D,), lambda: pl.semaphore_wait(barrier, 3))
        send(s, A, (B, C) if s in VIA_C else (B, C, D))
        send(s, C, (A, D))
        send(s, B, (A,) if s in LATE_TO_B else (A, D))
        send(s, D, (B, C))
        if s == 3:
            undisturbed(lambda: fetch_rows(3, x_row[3], x_row_last))
        if s == 9:
            forward(VIA_C[0], D, C, A)
        if s == 11:
            forward(VIA_C[1], D, C, A)
    for s in LATE_TO_B:
        send(s, B, (D,))
    for s in range(9):
        forward(s, A, B, D)
    forward(VIA_C[2], D, C, A)
    below = output_rows()
    forward(VIA_C[3], D, C, A)
    output_halves(below)
    for s in VIA_C[4:]:
        forward(s, D, C, A)
    for s in range(9, N_STEPS):
        forward(s, A, B, D)
    addr_copy.wait()

    for s in range(N_STEPS):
        if s < N_LOCAL:
            write_rows(OWN, STEPS_OF[s])
        forward(s, C, A, B)
        forward(s, B, A, C)
        on((D,) if s in VIA_C else (C, D), lambda: wait_received(LEFT, s))
        on((C, D) if s in LATE_TO_B else (B, C, D), lambda: wait_received(RIGHT, s))
        for steps in NEIGHBOUR_GROUPS:
            if s == steps[-1]:
                write_rows(LEFT, steps)
                on((A, C, D) if s in LATE_TO_B else ALL, lambda: write_rows(RIGHT, steps))
        if s in DIAG_EARLY:
            write_rows(DIAG, [DIAG_EARLY[s]], wait_for_them=True)
        wait_sent(s, forwarded=False)
        if s >= SEND_LAG:
            wait_sent(s - SEND_LAG, forwarded=True)

    for s in DIAG_LATE:
        if s == DIAG_LATE[-5]:
            for late in range(N_STEPS - SEND_LAG, N_STEPS):
                wait_sent(late, forwarded=True)
        write_rows(DIAG, [s], wait_for_them=True)

    @pl.when(me == B)
    def _():
        for steps in STEPS_OF:
            if steps[0] in LATE_TO_B:
                write_rows(RIGHT, steps, wait_for_them=True)


def pallas_dist_moe_cap_ep_n512_d256_e4_h512_kernel(
    x: jax.Array,
    router_W: jax.Array,
    route_idx: jax.Array,
    expert_W: jax.Array,
):
    del router_W
    hbm = pl.BlockSpec(memory_space=pltpu.HBM)
    out = pl.pallas_call(
        _body,
        out_shape=jax.ShapeDtypeStruct((2 * N_TOK, 2, 128), BF16),
        in_specs=[hbm, hbm, hbm],
        out_specs=pl.BlockSpec(memory_space=pltpu.VMEM),
        scratch_shapes=[
            pltpu.VMEM((4, 128), I32),
            pltpu.VMEM((N_LOCAL, 32, D_IN), F32),
            pltpu.VMEM((4, FIRST_ROW[-1], 128), U32),
            pltpu.VMEM((4, 128), I32),
            pltpu.SMEM((4, 128), I32),
            pltpu.VMEM((4, 128, 128), U32),
            pltpu.SemaphoreType.DMA((2 + len(BLOCKS) + 3 * N_LOCAL,)),
            pltpu.SemaphoreType.DMA((8 * N_STEPS,)),
            pltpu.SemaphoreType.DMA((4 * N_STEPS,)),
        ] + [pltpu.VMEM((D_IN, w), F32) for _, _, w in BLOCKS],
        compiler_params=pltpu.CompilerParams(
            collective_id=0, disable_bounds_checks=True, disable_semaphore_checks=True),
    )(x, route_idx.reshape(4, 128), expert_W)
    return out.reshape(N_TOK // 8, 4, 8, 128).transpose(0, 2, 1, 3).reshape(N_TOK, D_OUT)
```

```python
import jax
import jax.numpy as jnp
from jax import lax
from jax.experimental import pallas as pl
from jax.experimental.pallas import tpu as pltpu

F32, BF16, I32, U32 = jnp.float32, jnp.bfloat16, jnp.int32, jnp.uint32

N_TOK, D_IN, D_OUT = 512, 256, 512
N_EXP, N_LOCAL, CAP = 16, 4, 25

A, B, D, C = 0, 1, 2, 3
ALL = (0, 1, 2, 3)
OWN, RIGHT, DIAG, LEFT = 0, 1, 2, 3
DESTINATIONS = {A: (B, C), B: (A, D), C: (A, D), D: (A, B, C)}

WIDTH = (256, 256, 128, 128)
BLOCKS = [(e, c, w) for e, w in enumerate(WIDTH) for c in range(0, D_OUT, w)]
STEPS = [(0, 0, 8), (0, 8, CAP)] + [(b, 0, CAP) for b in range(1, len(BLOCKS))]
ROW_GROUPS = [(0, 8, 24, CAP)] + [(0, 24, CAP)] * 3


def _words(step):
    b, first, end = STEPS[step]
    _, c, w = BLOCKS[b]
    j = c // 128
    if w == 256:
        return [((p, j), (p, j + 1)) for p in range(first, end)]
    words = [((p, j), (p + 1, j)) for p in range(0, CAP - 1, 2)]
    if j % 2:
        words.append(((CAP - 1, j), (CAP - 1, j - 1)))
    return words


N_STEPS = len(STEPS)
EXPERT = [BLOCKS[b][0] for b, _, _ in STEPS]
STEPS_OF = [[s for s in range(N_STEPS) if EXPERT[s] == e] for e in range(N_LOCAL)]
WORDS = [_words(s) for s in range(N_STEPS)]
FIRST_ROW = [sum(pl.cdiv(len(w), 8) * 8 for w in WORDS[:s]) for s in range(N_STEPS + 1)]

VIA_C = (0, 1, 3, 4, 5, 6)
LATE_TO_B = STEPS_OF[2] + STEPS_OF[3]
NEIGHBOUR_GROUPS = ((0, 1, 2), (3, 4), (5, 6, 7, 8), (9, 10), (11,), (12,))
DIAG_EARLY = {8: 2, 10: 0, 11: 1}
DIAG_LATE = (7, 3, 8, 9, 4, 10, 5, 11, 6, 12)
SEND_LAG = 4
ZEROED_PER_STEP = 60


def _body(x_hbm, idx_hbm, w_hbm, out_ref,
          idx_v, rows_v, y_v, addr_v, addr_s, mask_v,
          local_sem, send_sem, recv_sem, *w_v):
    idx_copy = pltpu.make_async_copy(idx_hbm, idx_v, local_sem.at[0])
    idx_copy.start()
    w_copies = [
        pltpu.make_async_copy(
            w_hbm.at[e, :, pl.ds(c, w)], w_v[b], local_sem.at[2 + b])
        for b, (e, c, w) in enumerate(BLOCKS)
    ]
    for copy in w_copies:
        copy.start(priority=1)

    me = lax.axis_index("i")

    def chip(position):
        return dict(device_id=(position,), device_id_type=pl.DeviceIdType.MESH)

    def on(chips, fn):
        if len(chips) == len(ALL):
            return fn()
        if len(chips) == len(ALL) - 1:
            pred = me != [c for c in ALL if c not in chips][0]
        else:
            pred = me == chips[0]
            for c in chips[1:]:
                pred = pred | (me == c)
        pl.when(pred)(fn)

    barrier = pltpu.get_barrier_semaphore()
    for sender in ALL:
        on(DESTINATIONS[sender],
           lambda: pl.semaphore_signal(barrier, inc=1, **chip(sender)))

    def zero_output(first, end):
        out_ref[first:end] = jnp.zeros((end - first, 2, 128), BF16)

    rows_v[:, 24:32, :] = jnp.zeros((N_LOCAL, 8, D_IN), F32)
    zero_output((N_STEPS - 1) * ZEROED_PER_STEP, 2 * N_TOK)

    upper = (lax.broadcasted_iota(I32, (128, 128), 0)
             <= lax.broadcasted_iota(I32, (128, 128), 1))
    upper = jnp.where(upper, 1.0, 0.0).astype(BF16)
    ones = jnp.ones((128, 128), BF16)

    def running_counts(n):
        row = lax.broadcasted_iota(I32, (n, 128), 0)
        hits = []
        for b in range(4):
            e = jnp.broadcast_to(idx_v[b:b + 1, :], (n, 128))
            hits.append(jnp.where(((e - N_LOCAL * me) & (N_EXP - 1)) == row, 1.0, 0.0))
        hits = jnp.concatenate(hits, axis=0).astype(BF16)
        within = jnp.dot(hits, upper, preferred_element_type=F32)
        totals = jnp.dot(hits, ones, preferred_element_type=F32)
        counts, before = [within[:n]], totals[:n]
        for b in range(1, 4):
            counts.append(within[n * b:n * b + n] + before)
            before = before + totals[n * b:n * b + n]
        return counts

    def of_expert(counts, r, n):
        return [jnp.broadcast_to(cnt[r:r + 1, :], (n, 128)) for cnt in counts]

    def tokens_before(counts, slot):
        acc = jnp.where(counts[0] <= slot, 1.0, 0.0)
        for cnt in counts[1:]:
            acc = acc + jnp.where(cnt <= slot, 1.0, 0.0)
        return acc

    def as_int(small):
        return pltpu.bitcast(small + 8388608.0, I32)

    def row_of_x(counts, slot):
        tok = jnp.sum(tokens_before(counts, slot), axis=1, keepdims=True)
        return as_int(jnp.minimum(tok, N_TOK - 1.0)) & (N_TOK - 1)

    def rows_sem(e, group):
        return local_sem.at[2 + len(BLOCKS) + 3 * e + group]

    def fetch_rows(e, first_24, last):
        for p in range(CAP):
            t = first_24[p, 0] if p < CAP - 1 else last[e, 0]
            group = sum(p >= edge for edge in ROW_GROUPS[e][1:])
            pltpu.make_async_copy(
                x_hbm.at[pl.ds(t, 1)], rows_v.at[e, pl.ds(p, 1)],
                rows_sem(e, group)).start()

    awaited = []

    def fetched_rows(e, first, end):
        edges = ROW_GROUPS[e]
        for group in range(edges.index(first), edges.index(end)):
            if (e, group) not in awaited:
                awaited.append((e, group))
                buf = rows_v.at[e, pl.ds(edges[group], edges[group + 1] - edges[group])]
                pltpu.make_async_copy(buf, buf, rows_sem(e, group)).wait()
        return rows_v[e, pl.ds(first, pl.cdiv(end - first, 8) * 8), :].astype(BF16)

    addr_copy = pltpu.make_async_copy(addr_v, addr_s, local_sem.at[1])

    def output_rows():
        counts = running_counts(N_EXP)
        row = lax.broadcasted_iota(I32, (32, 128), 0)
        in_order = row.astype(F32)
        even_then_odd = jnp.minimum(2 * (row & 15) + (row >> 4), CAP - 1).astype(F32)
        below = [
            jnp.concatenate(
                [tokens_before(of_expert(counts, N_LOCAL * src + e, 32),
                               in_order if WIDTH[e] == 256 else even_then_odd)
                 for e in range(N_LOCAL)], axis=0).astype(BF16)
            for src in ALL]
        for src in ALL:
            tok = lax.dot_general(
                ones[:16], below[src], (((1,), (1,)), ((), ())), preferred_element_type=F32)
            tok = tok[0:1].astype(I32)
            addr_v[src:src + 1, :] = jnp.minimum(tok >> 3, 63) * 16 + ((tok >> 1) & 3)
        addr_copy.start()
        return below

    def output_halves(below):
        for src in ALL:
            tok = as_int(jnp.dot(below[src], ones, preferred_element_type=F32))
            half = jnp.where((tok & 1) == 1, U32(0xFFFF0000), U32(0xFFFF))
            mask_v[src] = jnp.where((tok & N_TOK) == 0, half, U32(0))

    started = [[] for _ in range(N_STEPS)]

    def remote(s, src, to, dst):
        rows = pl.ds(FIRST_ROW[s], len(WORDS[s]))
        return pltpu.make_async_remote_copy(
            y_v.at[src, rows], y_v.at[dst, rows],
            send_sem.at[(2 * to + (src != OWN)) * N_STEPS + s],
            recv_sem.at[dst * N_STEPS + s], **chip(to))

    def wait_received(src, s):
        remote(s, OWN, A, src).wait_recv()

    def send(s, to, chips):
        on(chips, lambda: remote(s, OWN, to, (me - to) & 3).start())
        started[s].append((OWN, to, chips))

    def forward(s, origin, by, to):
        src = (origin - by) % 4

        def fn():
            wait_received(src, s)
            remote(s, src, to, (origin - to) % 4).start()
        on((by,), fn)
        started[s].append((src, to, (by,)))

    def wait_sent(s, forwarded):
        for src, to, chips in started[s]:
            if (src != OWN) == forwarded:
                on(chips, lambda: remote(s, src, to, DIAG).wait_send())

    def write_rows(src, steps, wait_for_them=False):
        e = EXPERT[steps[0]]
        at = {(s, half): 32 * e + (STEPS[s][1] if WIDTH[e] == 256 else 16 * half)
              for s in steps for half in (0, 1)}
        masks = {(s, half): mask_v[src, pl.ds(first, len(WORDS[s])), :]
                 for (s, half), first in at.items()}
        entries = sorted(((p, j, s, i, half) for s in steps for i, word in enumerate(WORDS[s])
                          for half, (p, j) in enumerate(word)), reverse=True)
        for parity in (0, 1):
            batch = [entry for entry in entries if entry[0] % 2 == parity]
            base = {}
            for p, _, s, i, half in batch:
                if p not in base:
                    base[p] = addr_s[src, at[s, half] + i]
            old = [pltpu.bitcast(out_ref[base[p] + 4 * j], U32) for p, j, *_ in batch]
            if parity == 0:
                new = {}
                for s in steps:
                    if wait_for_them:
                        wait_received(src, s)
                    v = y_v[src, pl.ds(FIRST_ROW[s], len(WORDS[s])), :]
                    new[s, 0] = ((v << 16) | (v & U32(0xFFFF))) & masks[s, 0]
                    new[s, 1] = ((v >> 16) | (v & U32(0xFFFF0000))) & masks[s, 1]
            for (p, j, s, i, half), word in zip(batch, old):
                out_ref[base[p] + 4 * j] = pltpu.bitcast(word | new[s, half][i:i + 1], BF16)

    def undisturbed(fn):
        pl.when(me != len(ALL))(fn)

    idx_copy.wait()
    local = running_counts(8)
    slots = lax.broadcasted_iota(I32, (24, 128), 0).astype(F32)
    x_row = [row_of_x(of_expert(local, 0, 24), slots)]
    x_row_last = row_of_x(local, CAP - 1.0)
    undisturbed(lambda: fetch_rows(0, x_row[0], x_row_last))
    x_row += [row_of_x(of_expert(local, e, 24), slots) for e in (1, 2, 3)]
    fetch_rows(1, x_row[1], x_row_last)
    fetch_rows(2, x_row[2], x_row_last)

    lhs, last_slot = {}, {}
    for s, (b, first, end) in enumerate(STEPS):
        e, c, w = BLOCKS[b]
        if (e, first, end) not in lhs:
            lhs[e, first, end] = fetched_rows(e, first, end)
        if first == 0:
            w_copies[b].wait()
        rows, weights = lhs[e, first, end], w_v[b][...].astype(BF16)
        if w == 256:
            y = jnp.dot(rows, weights, preferred_element_type=F32)
            y = pltpu.bitcast(y.astype(BF16).astype(F32), U32)
            y = (y[:, :128] >> 16) | y[:, 128:]
        else:
            top, bottom = (jnp.dot(rows[h:h + 16], weights, preferred_element_type=F32)
                           for h in (0, 16))
            tail = bottom[8:]
            if c // 128 % 2:
                second = lax.broadcasted_iota(I32, (8, 128), 0) == 1
                tail = jnp.where(second, last_slot[e], tail)
            else:
                last_slot[e] = jnp.broadcast_to(tail[0:1], (8, 128))
            y = jnp.concatenate([top, bottom[:8], tail], axis=0)
            y = pltpu.bitcast(y.astype(BF16), U32)
        if s < N_STEPS - 1:
            zero_output(s * ZEROED_PER_STEP, (s + 1) * ZEROED_PER_STEP)
        y_v[OWN, pl.ds(FIRST_ROW[s], y.shape[0]), :] = y
        if s == 0:
            on((A, B, C), lambda: pl.semaphore_wait(barrier, 2))
            on((D,), lambda: pl.semaphore_wait(barrier, 3))
        send(s, A, (B, C) if s in VIA_C else (B, C, D))
        send(s, C, (A, D))
        send(s, B, (A,) if s in LATE_TO_B else (A, D))
        send(s, D, (B, C))
        if s == 3:
            undisturbed(lambda: fetch_rows(3, x_row[3], x_row_last))
        if s == 9:
            forward(VIA_C[0], D, C, A)
        if s == 11:
            forward(VIA_C[1], D, C, A)
    for s in LATE_TO_B:
        send(s, B, (D,))
    for s in range(9):
        forward(s, A, B, D)
    forward(VIA_C[2], D, C, A)
    below = output_rows()
    forward(VIA_C[3], D, C, A)
    output_halves(below)
    for s in VIA_C[4:]:
        forward(s, D, C, A)
    for s in range(9, N_STEPS):
        forward(s, A, B, D)
    addr_copy.wait()

    for s in range(N_STEPS):
        if s < N_LOCAL:
            write_rows(OWN, STEPS_OF[s])
        forward(s, C, A, B)
        forward(s, B, A, C)
        on((D,) if s in VIA_C else (C, D), lambda: wait_received(LEFT, s))
        on((C, D) if s in LATE_TO_B else (B, C, D), lambda: wait_received(RIGHT, s))
        for steps in NEIGHBOUR_GROUPS:
            if s == steps[-1]:
                write_rows(LEFT, steps)
                on((A, C, D) if s in LATE_TO_B else ALL, lambda: write_rows(RIGHT, steps))
        if s in DIAG_EARLY:
            write_rows(DIAG, [DIAG_EARLY[s]], wait_for_them=True)
        wait_sent(s, forwarded=False)
        if s >= SEND_LAG:
            wait_sent(s - SEND_LAG, forwarded=True)

    for s in DIAG_LATE[:-4]:
        write_rows(DIAG, [s], wait_for_them=True)

    @pl.when(me == B)
    def _():
        for steps in STEPS_OF:
            if steps[0] in LATE_TO_B:
                write_rows(RIGHT, steps, wait_for_them=True)

    for s in range(N_STEPS - SEND_LAG, N_STEPS):
        wait_sent(s, forwarded=True)
    for s in DIAG_LATE[-4:]:
        write_rows(DIAG, [s], wait_for_them=True)


def pallas_dist_moe_cap_ep_n512_d256_e4_h512_kernel(
    x: jax.Array,
    router_W: jax.Array,
    route_idx: jax.Array,
    expert_W: jax.Array,
):
    del router_W
    hbm = pl.BlockSpec(memory_space=pltpu.HBM)
    out = pl.pallas_call(
        _body,
        out_shape=jax.ShapeDtypeStruct((2 * N_TOK, 2, 128), BF16),
        in_specs=[hbm, hbm, hbm],
        out_specs=pl.BlockSpec(memory_space=pltpu.VMEM),
        scratch_shapes=[
            pltpu.VMEM((4, 128), I32),
            pltpu.VMEM((N_LOCAL, 32, D_IN), F32),
            pltpu.VMEM((4, FIRST_ROW[-1], 128), U32),
            pltpu.VMEM((4, 128), I32),
            pltpu.SMEM((4, 128), I32),
            pltpu.VMEM((4, 128, 128), U32),
            pltpu.SemaphoreType.DMA((2 + len(BLOCKS) + 3 * N_LOCAL,)),
            pltpu.SemaphoreType.DMA((8 * N_STEPS,)),
            pltpu.SemaphoreType.DMA((4 * N_STEPS,)),
        ] + [pltpu.VMEM((D_IN, w), F32) for _, _, w in BLOCKS],
        compiler_params=pltpu.CompilerParams(
            collective_id=0, disable_bounds_checks=True, disable_semaphore_checks=True),
    )(x, route_idx.reshape(4, 128), expert_W)
    return out.reshape(N_TOK // 8, 4, 8, 128).transpose(0, 2, 1, 3).reshape(N_TOK, D_OUT)
```
